```python
import numpy as np

kernel_name = "dist_rs_xy_x_m65536_n1024"

def setup_inputs():
    return {"x": np.random.randn(2, 65536, 1024).astype(np.float32)}

def reference(x: np.ndarray) -> np.ndarray:
    return x.sum(axis=0)
```

```python
import jax
import jax.numpy as jnp
from jax import lax
from jax.experimental import pallas as pl
from jax.experimental.pallas import tpu as pltpu


def make_kernel(C=64, D=3, E=1, P=6, nochk=False, interpret=False):
    def fn(x):
        _, m, n2 = x.shape
        n = n2 // 2
        half = m // 2
        nc = half // C
        nx, ny = nc + E, nc - E
        KX = 2 * D + 1
        KS = D + 2
        KL = P + 1

        def body(x_hbm, o_ref, lbuf, sbuf, abuf, lsem, asem, xs_sem, xr_sem, ys_sem, yr_sem):
            mx, my = lax.axis_index("x"), lax.axis_index("y")
            xpeer, ypeer = (1 - mx, my), (mx, 1 - my)
            mine = pl.ds(pl.multiple_of(mx * n, n), n)
            theirs = pl.ds(pl.multiple_of((1 - mx) * n, n), n)

            def rows(j):
                start = jnp.where(j < nc, my * half + j * C, (1 - my) * half + (j - E) * C)
                return pl.ds(pl.multiple_of(start, C), C)

            def load_s(j):
                return pltpu.make_async_copy(x_hbm.at[0, rows(j), theirs], lbuf.at[j % KL], lsem.at[j % KL])

            def load_a(j):
                return pltpu.make_async_copy(x_hbm.at[0, rows(j), mine], abuf.at[j % KL], asem.at[j % KL])

            def send_x(j):
                return pltpu.make_async_remote_copy(
                    sbuf.at[j % KS], o_ref.at[rows(j)], xs_sem.at[j % KS], xr_sem.at[j % KX],
                    device_id=xpeer, device_id_type=pl.DeviceIdType.MESH)

            def send_y(r):
                return pltpu.make_async_remote_copy(
                    o_ref.at[r], o_ref.at[r], ys_sem, yr_sem,
                    device_id=ypeer, device_id_type=pl.DeviceIdType.MESH)

            def convert(j):
                load_s(j).wait()
                sbuf[j % KS] = lbuf[j % KL].astype(jnp.bfloat16)

            barrier = pltpu.get_barrier_semaphore()
            for peer in (xpeer, ypeer):
                pl.semaphore_signal(barrier, 1, device_id=peer, device_id_type=pl.DeviceIdType.MESH)
            for j in range(KL):
                load_s(j).start()
            convert(0)
            pl.semaphore_wait(barrier, 2)
            send_x(0).start()
            load_a(0).start()
            load_s(KL).start()
            for j in range(1, D + 1):
                convert(j)
                if j < D:
                    send_x(j).start()
                load_s(j + KL).start()
            for j in range(1, KL):
                load_a(j).start()

            @pl.loop(0, nx)
            def _(k):
                load_a(k).wait()
                send_x(k).wait_recv()
                o_ref[rows(k), :] = (abuf[k % KL] + o_ref[rows(k), :].astype(jnp.float32)).astype(jnp.bfloat16)

                @pl.when(k < ny)
                def _():
                    send_y(rows(k)).start()

                @pl.when(k + D < nx)
                def _():
                    send_x(k + D).start()

                @pl.when(k + KL < nx)
                def _():
                    load_a(k + KL).start()

                c = k + D + 1

                @pl.when(c < nx)
                def _():
                    @pl.when(c >= KS)
                    def _():
                        send_x(c - KS).wait_send()
                    convert(c)

                    @pl.when(c + KL < nx)
                    def _():
                        load_s(c + KL).start()

            for j in range(nx - KS, nx):
                send_x(j).wait_send()
            send_y(pl.ds(pl.multiple_of(my * half, C), ny * C)).wait_send()
            send_y(pl.ds(pl.multiple_of((1 - my) * half, C), ny * C)).wait_recv()

        dma = pltpu.SemaphoreType.DMA
        return pl.pallas_call(
            body,
            out_shape=pltpu.VMEM((m, n), jnp.bfloat16),
            in_specs=[pl.BlockSpec(memory_space=pl.ANY)],
            out_specs=pl.BlockSpec(memory_space=pltpu.VMEM),
            scratch_shapes=[
                pltpu.VMEM((KL, C, n), jnp.float32),
                pltpu.VMEM((KS, C, n), jnp.bfloat16),
                pltpu.VMEM((KL, C, n), jnp.float32),
                dma((KL,)), dma((KL,)), dma((KS,)), dma((KX,)), dma, dma,
            ],
            compiler_params=pltpu.CompilerParams(collective_id=0, vmem_limit_bytes=32 * 2**20, disable_semaphore_checks=nochk),
            interpret=interpret,
        )(x)

    return fn


pallas_dist_rs_xy_x_m65536_n1024_kernel = make_kernel(C=32, D=4, E=1)
```

```python
import jax
import jax.numpy as jnp
import numpy as np
from jax import lax
from jax.experimental import pallas as pl
from jax.experimental.pallas import tpu as pltpu

I32 = jnp.int32
TILE = (8, 128)

UNITS, UNIT_ROWS, UNIT_WORDS = 4, 64, 16
TICK_ROWS = UNITS * UNIT_ROWS
STACK = 5

HEADER = 4
NOTE = (1 << 20) - 1
UNIT_FIXED = 9
FIXED = UNITS * UNIT_FIXED
STREAM = HEADER + FIXED
CODED_SIZES = tuple(range(5, 16))
PLAIN_SIZE = UNITS * UNIT_WORDS - FIXED
PIECE = FIXED // 3
PLAIN_COPY = STREAM + CODED_SIZES[-1] + 1

REF_ABOVE_MEAN = 1027
SAMPLE_ROWS = 128
RATE_MARGIN = 0.055
RANK = (7, 5, 3, 0, 1, 2, 4, 6)

MAX_GROUP = 36
PREFETCH = 3
SEND_SLOTS, RECV_SLOTS, IN_FLIGHT = 2 * MAX_GROUP + 1, 4, 2


def _i32(v):
    return np.int32(v - (1 << 32) if v >= (1 << 31) else v)


MSB, LOW_BYTES, SIGNS = _i32(0x80000000), _i32(0x00FF00FF), _i32(0x80008000)
TO_RANK = _i32(sum((p ^ r) << (4 * p) for p, r in enumerate(RANK)))
FROM_RANK = _i32(sum((p ^ r) << (4 * r) for p, r in enumerate(RANK)))


def _shl(a, n):
    return lax.shift_left(a, jnp.broadcast_to(jnp.asarray(n, I32), a.shape))


def _shr(a, n):
    return lax.shift_right_logical(a, jnp.broadcast_to(jnp.asarray(n, I32), a.shape))


def _tile(v):
    return jnp.full(TILE, v, I32)


def _permute(table, v):
    return v ^ (_shr(jnp.full(v.shape, table), jnp.minimum(_shl(v, 2), 31)) & 7)


def _ranks(t):
    return [_permute(TO_RANK, _shr(t, s) & 31) for s in (8, 24)]


def _push(stack, n, top):
    m = 32 - n
    below = [_shr(b, n) | _shl(a, m) for a, b in zip(stack, stack[1:])]
    return [_shr(stack[0], n) | top] + below


def _pop(stack, n):
    m = 32 - n
    above = [_shl(a, n) | _shr(b, m) for a, b in zip(stack, stack[1:])]
    return above + [_shl(stack[-1], n)]


def _pack_unit(words, ref, width, stack, drain):
    ts = [ref - w for w in words]
    fixed = [(a & LOW_BYTES) | _shl(b & LOW_BYTES, 8) for a, b in zip(ts[::2], ts[1::2])]
    signs = None
    for i in range(0, UNIT_WORDS, 2):
        code = bits = None
        for q in _ranks(ts[i]) + _ranks(ts[i + 1]):
            code = _shr(jnp.full(q.shape, MSB) if code is None else _shr(code, 1) | MSB, q)
            bits = q + 4 if bits is None else bits + q
        stack = _push(stack, jnp.minimum(bits, 31), code)
        if i % 4 == 2:
            drain(i // 4, stack[0])
            stack = _pop(stack, width)
        for t in ts[i : i + 2]:
            signs = t & SIGNS if signs is None else _shr(signs, 1) | (t & SIGNS)
    return fixed + [signs], stack


def _unpack_unit(fixed, ref, width, stack, refill):
    signs, words = fixed[-1], []
    for i in reversed(range(0, UNIT_WORDS, 2)):
        if i % 4 == 2:
            stack = _push(stack, width, refill(i // 4))
        code, bits, ps = stack[0] | 0b11110, 4, []
        for _ in range(4):
            q = lax.clz(code)
            code = _shl(_shl(code, 1), q)
            bits = bits + q
            ps.append(_permute(FROM_RANK, q))
        stack = _pop(stack, bits)
        for low, hi, lo in ((_shr(fixed[i // 2], 8), *ps[:2]), (fixed[i // 2], *ps[2:])):
            t = (low & LOW_BYTES) | _shl(lo, 8) | _shl(hi, 24) | (signs & SIGNS)
            words.insert(0, ref - t)
            signs = _shl(signs, 1)
    return words, stack


def _field(size, unit, j):
    width = 2 * jnp.minimum(size, CODED_SIZES[-1])
    bit = (4 * (UNITS - 1 - unit) + j) * width
    return STREAM + (bit >> 5), bit & 31, width


def _unpack_pair(messages, sizes, units, ref, stack):
    def refill(j):
        tops = []
        for message, size, unit in zip(messages, sizes, units):
            word, shift, width = _field(size, unit, j)
            two = message[pl.ds(word, 2)]
            top = _shl(two[0], shift) | _shr(_shr(two[1], 1), 31 - shift)
            tops.append(top & (MSB >> (width - 1)))
        return jnp.stack(tops)

    fixed = [m[pl.ds(HEADER + UNIT_FIXED * u, UNIT_FIXED)] for m, u in zip(messages, units)]
    fixed = [jnp.stack([f[i] for f in fixed]) for i in range(UNIT_FIXED)]
    width = jnp.stack([_tile(_field(size, 0, 0)[2]) for size in sizes])
    return _unpack_unit(fixed, ref, width, stack, refill)


def _reduce_scatter(x, interpret=False):
    _, m, n = x.shape
    n //= 2
    ticks = m // 2 // TICK_ROWS
    assert n == 4 * TILE[1] and 2 * ticks * TICK_ROWS == m and ticks >= PREFETCH

    def packed_before(t, lib=jnp):
        ahead = lib.minimum(lib.minimum(2 * t, t + 1 + (t >> 1)), t + MAX_GROUP)
        return lib.clip(lib.maximum(ahead, t + 1), 0, ticks)

    starts = [0]
    while starts[-1] < ticks:
        starts.append(int(packed_before(starts[-1], np)))

    def group(t):
        first, end = starts[:2]
        for lo, hi in zip(starts[1:], starts[2:]):
            first, end = jnp.where(t >= lo, lo, first), jnp.where(t >= lo, hi, end)
        return first, end

    def opens(t):
        return group(t)[0] == t

    def mirror(t):
        first, end = group(t)
        return first + end - 1 - t

    def at(ring, t):
        return lax.rem(t, jnp.int32(ring))

    def rows(start, size):
        return pl.ds(pl.multiple_of(jnp.asarray(start, I32), UNIT_ROWS), size)

    def body(x_hbm, out, src, x_own, y_own, send, x_recv, y_recv, packer, stacks, unpacker, sizes,
             src_sem, x_own_sem, y_own_sem, x_send_sem, x_recv_sem, y_send_sem, y_recv_sem):
        my_x, my_y = lax.axis_index("x"), lax.axis_index("y")
        x_peer, y_peer = (1 - my_x, my_y), (my_x, 1 - my_y)
        my_cols = pl.ds(pl.multiple_of(my_x * n, n), n)
        peer_cols = pl.ds(pl.multiple_of((1 - my_x) * n, n), n)
        x_rows, y_rows = my_y * (m // 2), (1 - my_y) * (m // 2)
        sides = (x_rows, x_own, x_own_sem), (y_rows, y_own, y_own_sem)
        SENT, FROM_X, FROM_Y = range(3)

        def load(t, cols, first_row, buf, sem):
            slot = at(PREFETCH, t)
            return pltpu.make_async_copy(
                x_hbm.at[0, rows(first_row, TICK_ROWS), cols], buf.at[slot], sem.at[slot])

        def src_load(e):
            return load(e, peer_cols, x_rows + mirror(e) * TICK_ROWS, src, src_sem)

        def own_load(t, base, buf, sem):
            return load(t, my_cols, base + t * TICK_ROWS, buf, sem)

        def x_copy(t, piece, start, count, offset=0):
            return pltpu.make_async_remote_copy(
                send.at[at(SEND_SLOTS, mirror(t)), pl.ds(offset + start, count)],
                x_recv.at[at(RECV_SLOTS, t), pl.ds(start, count)],
                x_send_sem.at[2 * at(IN_FLIGHT, t) + piece // 3],
                x_recv_sem.at[4 * at(RECV_SLOTS, t) + piece],
                device_id=x_peer, device_id_type=pl.DeviceIdType.MESH)

        def y_copy(t, piece, start, count):
            return pltpu.make_async_remote_copy(
                x_recv.at[at(RECV_SLOTS, t), pl.ds(start, count)],
                y_recv.at[at(RECV_SLOTS, t), pl.ds(start, count)],
                y_send_sem.at[2 * at(IN_FLIGHT, t) + piece // 3],
                y_recv_sem.at[2 * at(RECV_SLOTS, t) + piece // 3],
                device_id=y_peer, device_id_type=pl.DeviceIdType.MESH)

        def head_part(t, count, action):
            lax.cond(opens(t), lambda: action(0, 0, HEADER + count), lambda: action(0, HEADER, count))

        def stream_part(size, action, options=(*CODED_SIZES, PLAIN_SIZE)):
            if len(options) == 1:
                return action(3, STREAM, options[0])
            low, high = options[: len(options) // 2], options[len(options) // 2 :]
            lax.cond(size < high[0], lambda: stream_part(size, action, low),
                     lambda: stream_part(size, action, high))

        def pack(e):
            first, end = group(e)
            message = send.at[at(SEND_SLOTS, e)]

            def rounded(start, size):
                values = src[at(PREFETCH, e), rows(start, size), :]
                return pltpu.bitcast(values.astype(jnp.bfloat16), I32)

            src_load(e).wait()

            @pl.when(e == first)
            def _():
                w = rounded(0, SAMPLE_ROWS)
                total = jnp.sum((w[:16] & 0x7FFF) + (_shr(w[:16], 16) & 0x7FFF), keepdims=True)
                ref = jnp.broadcast_to(jnp.minimum((total >> 14) + REF_ABOVE_MEAN, 0x7FFF), TILE)
                ref = ref | _shl(ref, 16)
                lo, hi = _ranks(jnp.tile(ref, (SAMPLE_ROWS // 16, 4)) - w)
                bits = jnp.sum(lo + hi) + int(SAMPLE_ROWS * n * (1 + RATE_MARGIN))
                size = ((bits * (TICK_ROWS // SAMPLE_ROWS)) >> 15) + 1
                sizes[SENT, first] = jnp.clip(size, CODED_SIZES[0], CODED_SIZES[-1])
                packer[...] = jnp.stack([ref] + [_tile(0)] * (STACK + 1))

            size, state = sizes[SENT, first], packer[...]
            ref = state[0]
            stacks[UNITS] = state[1:-1]
            message[STREAM + size] = _tile(0)

            def pack_unit(i, carry):
                u, partial = UNITS - 1 - i, [carry[0]]

                def drain(j, top):
                    word, shift, width = _field(size, u, j)
                    top = top & (MSB >> (width - 1))
                    filled = partial[0] | _shr(top, shift)
                    message[word] = filled
                    rest = _shl(_shl(top, 1), 31 - shift)
                    partial[0] = jnp.where(_tile(shift + width) >= 32, rest, filled)

                w = rounded(u * UNIT_ROWS, UNIT_ROWS)
                words = [w[r : r + 8, c : c + 128] for r in range(0, 32, 8) for c in range(0, n, 128)]
                message[pl.ds(PLAIN_COPY + HEADER + u * UNIT_WORDS, UNIT_WORDS)] = jnp.stack(words)
                fixed, stack = _pack_unit(words, ref, _tile(2 * size), carry[1], drain)
                message[pl.ds(HEADER + u * UNIT_FIXED, UNIT_FIXED)] = jnp.stack(fixed)
                stacks[u] = jnp.stack(stack)
                return partial[0], stack

            start = _tile(0), [state[1 + i] for i in range(STACK)]
            _, stack = lax.fori_loop(0, UNITS, pack_unit, start, unroll=True)

            @pl.when(e + PREFETCH < ticks)
            def _():
                src_load(e + PREFETCH).start()

            def check_pair(i, mismatch):
                u = 2 * i
                seen = stacks[pl.ds(u, 3)]
                plain = message[pl.ds(PLAIN_COPY + HEADER + u * UNIT_WORDS, 2 * UNIT_WORDS)]
                got_words, got_stack = _unpack_pair(
                    (message, message), (size, size), (u, u + 1), jnp.stack([ref, ref]),
                    [seen[0:2, k] for k in range(STACK)])
                for j in range(2):
                    for k in reversed(range(UNIT_WORDS)):
                        mismatch = mismatch | (got_words[k][j] ^ plain[j * UNIT_WORDS + k])
                    for k in range(STACK):
                        mismatch = mismatch | (got_stack[k][j] ^ seen[j + 1, k])
                return mismatch

            mismatch = lax.fori_loop(0, UNITS // 2, check_pair, state[-1], unroll=True)
            packer[...] = jnp.stack([ref] + stack + [mismatch])

            @pl.when(e == end - 1)
            def _():
                note = (ref & 0x7FFF) | _tile(size << 15)
                message[0:HEADER] = jnp.stack(stack[: HEADER - 1] + [stack[HEADER - 1] | note])
                message[PLAIN_COPY : PLAIN_COPY + HEADER] = jnp.stack([_tile(PLAIN_SIZE << 15)] * HEADER)
                lost = mismatch | (stack[HEADER - 1] & NOTE)
                for word in stack[HEADER:]:
                    lost = lost | word
                exact = jnp.max(jnp.where(lost != 0, 1, 0)) == 0
                sizes[SENT, first] = jnp.where(exact, size, PLAIN_SIZE)

        def start_send(t):
            size = sizes[SENT, group(t)[0]]
            offset = jnp.where(size == PLAIN_SIZE, PLAIN_COPY, 0)
            head_part(t, PIECE, lambda *part: x_copy(t, *part, offset).start())
            for piece in (1, 2):
                x_copy(t, piece, HEADER + piece * PIECE, PIECE, offset).start()
            stream_part(size, lambda *part: x_copy(t, *part, offset).start())

        def relay(t, *part):
            x_copy(t, *part).wait_recv()
            y_copy(t, *part).start()

        def received_size(row, recv, t):
            @pl.when(opens(t))
            def _():
                sizes[row, t] = jnp.max((recv[at(RECV_SLOTS, t), HEADER - 1] & NOTE) >> 15)

            return sizes[row, group(t)[0]]

        def reduce(t, both_sizes):
            messages = [recv.at[at(RECV_SLOTS, t)] for recv in (x_recv, y_recv)]

            @pl.when(opens(t))
            def _():
                head = jnp.stack([message[0:HEADER] for message in messages], axis=1)
                ref = head[-1] & 0x7FFF
                stack = [head[i] for i in range(HEADER - 1)] + [head[-1] & ~NOTE]
                stack += [jnp.zeros_like(ref)] * (STACK - HEADER)
                unpacker[...] = jnp.stack([ref | _shl(ref, 16)] + stack)

            for side in sides:
                own_load(t, *side).wait()
            state = unpacker[...]
            ref = state[0]

            def reduce_unit(u, stack):
                words, stack = _unpack_pair(messages, both_sizes, (u, u), ref, stack)
                for j, (base, own, _) in enumerate(sides):
                    plain = messages[j][pl.ds(HEADER + u * UNIT_WORDS, UNIT_WORDS)]
                    is_plain = _tile(both_sizes[j]) == PLAIN_SIZE
                    w = [jnp.where(is_plain, plain[i], words[i][j]) for i in range(UNIT_WORDS)]
                    w = jnp.concatenate([jnp.concatenate(w[i : i + 4], axis=1) for i in range(0, 16, 4)])
                    other = pltpu.bitcast(w, jnp.bfloat16).astype(jnp.float32)
                    total = own[at(PREFETCH, t), rows(u * UNIT_ROWS, UNIT_ROWS), :] + other
                    out[rows(base + t * TICK_ROWS + u * UNIT_ROWS, UNIT_ROWS), :] = total.astype(out.dtype)
                return stack

            stack = lax.fori_loop(0, UNITS, reduce_unit, [state[1 + i] for i in range(STACK)], unroll=True)
            unpacker[...] = jnp.stack([ref] + stack)

            @pl.when(t + PREFETCH < ticks)
            def _():
                for side in sides:
                    own_load(t + PREFETCH, *side).start()

        @pl.loop(0, PREFETCH)
        def _(e):
            src_load(e).start()

        for recv in (x_recv, y_recv):
            recv[:, STREAM:] = jnp.zeros((RECV_SLOTS, PLAIN_SIZE, *TILE), I32)
        barrier = pltpu.get_barrier_semaphore()
        for peer in (x_peer, y_peer):
            pl.semaphore_signal(barrier, 1, device_id=peer, device_id_type=pl.DeviceIdType.MESH)

        @pl.loop(-2, ticks + 1)
        def _(step):
            relaying = (step >= 0) & (step < ticks)

            @pl.when(relaying)
            def _():
                head_part(step, PIECE, lambda *part: relay(step, *part))

            @pl.when(step == -1)
            def _():
                pl.semaphore_wait(barrier, 2)

            @pl.when((step >= -1) & (step + 1 < ticks))
            def _():
                start_send(step + 1)

            @pl.when(step == -1)
            def _():
                @pl.loop(0, PREFETCH)
                def _(t):
                    for side in sides:
                        own_load(t, *side).start()

            @pl.loop(0, 2)
            def _(i):
                e = packed_before(step + 1) + i
                pl.when(e < packed_before(step + 2))(lambda: pack(e))
                pl.when(relaying)(lambda: relay(step, 1 + i, HEADER + (1 + i) * PIECE, PIECE))

            @pl.when(relaying)
            def _():
                stream_part(received_size(FROM_X, x_recv, step), lambda *part: relay(step, *part))

            @pl.when(step >= 1)
            def _():
                t = step - 1
                head_part(t, FIXED, lambda *part: y_copy(t, *part).wait())
                x_size, y_size = sizes[FROM_X, group(t)[0]], received_size(FROM_Y, y_recv, t)
                stream_part(y_size, lambda *part: y_copy(t, *part).wait_recv())
                reduce(t, (x_size, y_size))
                stream_part(x_size, lambda *part: y_copy(t, *part).wait_send())

            @pl.when(relaying)
            def _():
                head_part(step, FIXED, lambda *part: x_copy(step, *part).wait_send())
                stream_part(sizes[SENT, group(step)[0]], lambda *part: x_copy(step, *part).wait_send())

    vmem, dma = pltpu.VMEM, pltpu.SemaphoreType.DMA
    staging = vmem((PREFETCH, TICK_ROWS, n), jnp.float32)
    received = vmem((RECV_SLOTS, STREAM + PLAIN_SIZE, *TILE), I32)
    return pl.pallas_call(
        body,
        out_shape=vmem((m, n), jnp.bfloat16),
        in_specs=[pl.BlockSpec(memory_space=pl.ANY)],
        out_specs=pl.BlockSpec(memory_space=vmem),
        scratch_shapes=[
            staging, staging, staging,
            vmem((SEND_SLOTS, PLAIN_COPY + STREAM + PLAIN_SIZE, *TILE), I32),
            received, received,
            vmem((STACK + 2, *TILE), I32),
            vmem((UNITS + 1, STACK, *TILE), I32),
            vmem((STACK + 1, 2, *TILE), I32),
            pltpu.SMEM((3, ticks), I32),
            dma((PREFETCH,)), dma((PREFETCH,)), dma((PREFETCH,)),
            dma((2 * IN_FLIGHT,)), dma((4 * RECV_SLOTS,)),
            dma((2 * IN_FLIGHT,)), dma((2 * RECV_SLOTS,)),
        ],
        compiler_params=pltpu.CompilerParams(collective_id=0, vmem_limit_bytes=52 * 2**20),
        interpret=interpret,
    )(x)


def pallas_dist_rs_xy_x_m65536_n1024_kernel(x: jax.Array):
    return _reduce_scatter(x)
```

```python
import jax
import jax.numpy as jnp
import numpy as np
from jax import lax
from jax.experimental import pallas as pl
from jax.experimental.pallas import tpu as pltpu

I32 = jnp.int32
TILE = (8, 128)

UNITS, UNIT_ROWS, UNIT_WORDS = 4, 64, 16
TICK_ROWS = UNITS * UNIT_ROWS
STACK = 5

HEADER = 4
NOTE = (1 << 20) - 1
UNIT_FIXED = 9
FIXED = UNITS * UNIT_FIXED
STREAM = HEADER + FIXED
CODED_SIZES = tuple(range(5, 16))
PLAIN_SIZE = UNITS * UNIT_WORDS - FIXED
PIECE = FIXED // 3
PLAIN_COPY = STREAM + CODED_SIZES[-1] + 1

REF_ABOVE_MEAN = 771
SAMPLE_ROWS = 64
RATE_MARGIN = 0.055
RANK = (7, 3, 0, 1, 2, 4, 5, 6)

MAX_GROUP = 36
PREFETCH = 3
SEND_SLOTS, RECV_SLOTS, IN_FLIGHT = 2 * MAX_GROUP + 1, 4, 2


def _i32(v):
    return np.int32(v - (1 << 32) if v >= (1 << 31) else v)


MSB, LOW_BYTES, SIGNS = _i32(0x80000000), _i32(0x00FF00FF), _i32(0x80008000)
TO_RANK = _i32(sum((p ^ r) << (4 * p) for p, r in enumerate(RANK)))
FROM_RANK = _i32(sum((p ^ r) << (4 * r) for p, r in enumerate(RANK)))


def _shl(a, n):
    return lax.shift_left(a, jnp.broadcast_to(jnp.asarray(n, I32), a.shape))


def _shr(a, n):
    return lax.shift_right_logical(a, jnp.broadcast_to(jnp.asarray(n, I32), a.shape))


def _tile(v):
    return jnp.full(TILE, v, I32)


def _permute(table, v):
    return v ^ (_shr(jnp.full(v.shape, table), jnp.minimum(_shl(v, 2), 31)) & 7)


def _ranks(t):
    return [_permute(TO_RANK, _shr(t, s) & 31) for s in (8, 24)]


def _push(stack, n, top):
    m = 32 - n
    below = [_shr(b, n) | _shl(a, m) for a, b in zip(stack, stack[1:])]
    return [_shr(stack[0], n) | top] + below


def _pop(stack, n):
    m = 32 - n
    above = [_shl(a, n) | _shr(b, m) for a, b in zip(stack, stack[1:])]
    return above + [_shl(stack[-1], n)]


def _pack_unit(words, ref, width, stack, drain):
    ts = [ref - w for w in words]
    fixed = [(a & LOW_BYTES) | _shl(b & LOW_BYTES, 8) for a, b in zip(ts[::2], ts[1::2])]
    signs = None
    for i in range(0, UNIT_WORDS, 2):
        code = bits = None
        for q in _ranks(ts[i]) + _ranks(ts[i + 1]):
            code = _shr(jnp.full(q.shape, MSB) if code is None else _shr(code, 1) | MSB, q)
            bits = q + 4 if bits is None else bits + q
        stack = _push(stack, jnp.minimum(bits, 31), code)
        if i % 4 == 2:
            drain(i // 4, stack[0])
            stack = _pop(stack, width)
        for t in ts[i : i + 2]:
            signs = t & SIGNS if signs is None else _shr(signs, 1) | (t & SIGNS)
    return fixed + [signs], stack


def _unpack_unit(fixed, ref, width, stack, refill):
    signs, words = fixed[-1], []
    for i in reversed(range(0, UNIT_WORDS, 2)):
        if i % 4 == 2:
            stack = _push(stack, width, refill(i // 4))
        code, bits, ps = stack[0] | 1, 4, []
        for _ in range(4):
            q = lax.clz(code)
            code = _shl(_shl(code, 1) | 1, q)
            bits = bits + q
            ps.append(_permute(FROM_RANK, q))
        stack = _pop(stack, jnp.minimum(bits, 31))
        for low, hi, lo in ((_shr(fixed[i // 2], 8), *ps[:2]), (fixed[i // 2], *ps[2:])):
            t = (low & LOW_BYTES) | _shl(lo, 8) | _shl(hi, 24) | (signs & SIGNS)
            words.insert(0, ref - t)
            signs = _shl(signs, 1)
    return words, stack


def _field(size, unit, j):
    width = 2 * jnp.minimum(size, CODED_SIZES[-1])
    bit = (4 * (UNITS - 1 - unit) + j) * width
    return STREAM + (bit >> 5), bit & 31, width


def _unpack_pair(messages, sizes, units, ref, stack):
    def refill(j):
        tops = []
        for message, size, unit in zip(messages, sizes, units):
            word, shift, width = _field(size, unit, j)
            two = message[pl.ds(word, 2)]
            top = _shl(two[0], shift) | _shr(_shr(two[1], 1), 31 - shift)
            tops.append(top & (MSB >> (width - 1)))
        return jnp.stack(tops)

    fixed = [m[pl.ds(HEADER + UNIT_FIXED * u, UNIT_FIXED)] for m, u in zip(messages, units)]
    fixed = [jnp.stack([f[i] for f in fixed]) for i in range(UNIT_FIXED)]
    width = jnp.stack([_tile(_field(size, 0, 0)[2]) for size in sizes])
    return _unpack_unit(fixed, ref, width, stack, refill)


def pallas_dist_rs_xy_x_m65536_n1024_kernel(x: jax.Array):
    _, m, n = x.shape
    n //= 2
    ticks = m // 2 // TICK_ROWS
    assert n == 4 * TILE[1] and 2 * ticks * TICK_ROWS == m and ticks >= PREFETCH

    def packed_before(t, lib=jnp):
        ahead = lib.minimum(lib.minimum(2 * t, t + 1 + (t >> 1)), t + MAX_GROUP)
        return lib.clip(lib.maximum(ahead, t + 1), 0, ticks)

    starts = [0]
    while starts[-1] < ticks:
        starts.append(int(packed_before(starts[-1], np)))

    def group(t):
        first, end = starts[:2]
        for lo, hi in zip(starts[1:], starts[2:]):
            first, end = jnp.where(t >= lo, lo, first), jnp.where(t >= lo, hi, end)
        return first, end

    def opens(t):
        return group(t)[0] == t

    def mirror(t):
        first, end = group(t)
        return first + end - 1 - t

    def at(ring, t):
        return lax.rem(t, jnp.int32(ring))

    def rows(start, size):
        return pl.ds(pl.multiple_of(jnp.asarray(start, I32), UNIT_ROWS), size)

    def body(x_hbm, out, src, x_own, y_own, send, x_recv, y_recv, packer, stacks, unpacker, sizes,
             src_sem, x_own_sem, y_own_sem, x_send_sem, x_recv_sem, y_send_sem, y_recv_sem):
        my_x, my_y = lax.axis_index("x"), lax.axis_index("y")
        x_peer, y_peer = (1 - my_x, my_y), (my_x, 1 - my_y)
        my_cols = pl.ds(pl.multiple_of(my_x * n, n), n)
        peer_cols = pl.ds(pl.multiple_of((1 - my_x) * n, n), n)
        x_rows, y_rows = my_y * (m // 2), (1 - my_y) * (m // 2)
        sides = (x_rows, x_own, x_own_sem), (y_rows, y_own, y_own_sem)
        SENT, FROM_X, FROM_Y = range(3)

        def load(t, cols, first_row, buf, sem):
            slot = at(PREFETCH, t)
            return pltpu.make_async_copy(
                x_hbm.at[0, rows(first_row, TICK_ROWS), cols], buf.at[slot], sem.at[slot])

        def src_load(e):
            return load(e, peer_cols, x_rows + mirror(e) * TICK_ROWS, src, src_sem)

        def own_load(t, base, buf, sem):
            return load(t, my_cols, base + t * TICK_ROWS, buf, sem)

        def x_copy(t, piece, start, count, offset=0):
            return pltpu.make_async_remote_copy(
                send.at[at(SEND_SLOTS, mirror(t)), pl.ds(offset + start, count)],
                x_recv.at[at(RECV_SLOTS, t), pl.ds(start, count)],
                x_send_sem.at[2 * at(IN_FLIGHT, t) + piece // 3],
                x_recv_sem.at[4 * at(RECV_SLOTS, t) + piece],
                device_id=x_peer, device_id_type=pl.DeviceIdType.MESH)

        def y_copy(t, piece, start, count):
            return pltpu.make_async_remote_copy(
                x_recv.at[at(RECV_SLOTS, t), pl.ds(start, count)],
                y_recv.at[at(RECV_SLOTS, t), pl.ds(start, count)],
                y_send_sem.at[2 * at(IN_FLIGHT, t) + piece // 3],
                y_recv_sem.at[2 * at(RECV_SLOTS, t) + piece // 3],
                device_id=y_peer, device_id_type=pl.DeviceIdType.MESH)

        def head_part(t, count, action):
            lax.cond(opens(t), lambda: action(0, 0, HEADER + count), lambda: action(0, HEADER, count))

        def stream_part(size, action, options=(*CODED_SIZES, PLAIN_SIZE)):
            if len(options) == 1:
                return action(3, STREAM, options[0])
            low, high = options[: len(options) // 2], options[len(options) // 2 :]
            lax.cond(size < high[0], lambda: stream_part(size, action, low),
                     lambda: stream_part(size, action, high))

        def pack(e):
            first, end = group(e)
            message = send.at[at(SEND_SLOTS, e)]

            def rounded(start, size):
                values = src[at(PREFETCH, e), rows(start, size), :]
                return pltpu.bitcast(values.astype(jnp.bfloat16), I32)

            src_load(e).wait()

            @pl.when(e == first)
            def _():
                w = rounded(0, SAMPLE_ROWS)
                total = jnp.sum((w[:16] & 0x7FFF) + (_shr(w[:16], 16) & 0x7FFF), keepdims=True)
                ref = jnp.broadcast_to(jnp.minimum((total >> 14) + REF_ABOVE_MEAN, 0x7FFF), TILE)
                ref = ref | _shl(ref, 16)
                lo, hi = _ranks(jnp.tile(ref, (SAMPLE_ROWS // 16, 4)) - w)
                bits = jnp.sum(lo + hi) + int(SAMPLE_ROWS * n * (1 + RATE_MARGIN))
                size = ((bits * (TICK_ROWS // SAMPLE_ROWS)) >> 15) + 1
                sizes[SENT, first] = jnp.clip(size, CODED_SIZES[0], CODED_SIZES[-1])
                packer[...] = jnp.stack([ref] + [_tile(0)] * (STACK + 1))

            size, state = sizes[SENT, first], packer[...]
            ref = state[0]
            stacks[UNITS] = state[1:-1]
            message[STREAM + size] = _tile(0)

            def pack_unit(i, carry):
                u, partial = UNITS - 1 - i, [carry[0]]

                def drain(j, top):
                    word, shift, width = _field(size, u, j)
                    top = top & (MSB >> (width - 1))
                    filled = partial[0] | _shr(top, shift)
                    message[word] = filled
                    rest = _shl(_shl(top, 1), 31 - shift)
                    partial[0] = jnp.where(_tile(shift + width) >= 32, rest, filled)

                w = rounded(u * UNIT_ROWS, UNIT_ROWS)
                words = [w[r : r + 8, c : c + 128] for r in range(0, 32, 8) for c in range(0, n, 128)]
                message[pl.ds(PLAIN_COPY + HEADER + u * UNIT_WORDS, UNIT_WORDS)] = jnp.stack(words)
                fixed, stack = _pack_unit(words, ref, _tile(2 * size), carry[1], drain)
                message[pl.ds(HEADER + u * UNIT_FIXED, UNIT_FIXED)] = jnp.stack(fixed)
                stacks[u] = jnp.stack(stack)
                return partial[0], stack

            start = _tile(0), [state[1 + i] for i in range(STACK)]
            _, stack = lax.fori_loop(0, UNITS, pack_unit, start, unroll=True)

            @pl.when(e + PREFETCH < ticks)
            def _():
                src_load(e + PREFETCH).start()

            def check_pair(i, mismatch):
                u = 2 * i
                seen = stacks[pl.ds(u, 3)]
                plain = message[pl.ds(PLAIN_COPY + HEADER + u * UNIT_WORDS, 2 * UNIT_WORDS)]
                got_words, got_stack = _unpack_pair(
                    (message, message), (size, size), (u, u + 1), jnp.stack([ref, ref]),
                    [seen[0:2, k] for k in range(STACK)])
                for j in range(2):
                    for k in reversed(range(UNIT_WORDS)):
                        mismatch = mismatch | (got_words[k][j] ^ plain[j * UNIT_WORDS + k])
                    for k in range(STACK):
                        mismatch = mismatch | (got_stack[k][j] ^ seen[j + 1, k])
                return mismatch

            mismatch = lax.fori_loop(0, UNITS // 2, check_pair, state[-1], unroll=True)
            packer[...] = jnp.stack([ref] + stack + [mismatch])

            @pl.when(e == end - 1)
            def _():
                note = (ref & 0x7FFF) | _tile(size << 15)
                message[0:HEADER] = jnp.stack(stack[: HEADER - 1] + [stack[HEADER - 1] | note])
                message[PLAIN_COPY : PLAIN_COPY + HEADER] = jnp.stack([_tile(PLAIN_SIZE << 15)] * HEADER)
                lost = mismatch | (stack[HEADER - 1] & NOTE)
                for word in stack[HEADER:]:
                    lost = lost | word
                exact = jnp.max(jnp.where(lost != 0, 1, 0)) == 0
                sizes[SENT, first] = jnp.where(exact, size, PLAIN_SIZE)

        def start_send(t):
            size = sizes[SENT, group(t)[0]]
            offset = jnp.where(size == PLAIN_SIZE, PLAIN_COPY, 0)
            head_part(t, PIECE, lambda *part: x_copy(t, *part, offset).start())
            for piece in (1, 2):
                x_copy(t, piece, HEADER + piece * PIECE, PIECE, offset).start()
            stream_part(size, lambda *part: x_copy(t, *part, offset).start())

        def relay(t, *part):
            x_copy(t, *part).wait_recv()
            y_copy(t, *part).start()

        def received_size(row, recv, t):
            @pl.when(opens(t))
            def _():
                sizes[row, t] = jnp.max((recv[at(RECV_SLOTS, t), HEADER - 1] & NOTE) >> 15)

            return sizes[row, group(t)[0]]

        def reduce(t, both_sizes):
            messages = [recv.at[at(RECV_SLOTS, t)] for recv in (x_recv, y_recv)]

            @pl.when(opens(t))
            def _():
                head = jnp.stack([message[0:HEADER] for message in messages], axis=1)
                ref = head[-1] & 0x7FFF
                stack = [head[i] for i in range(HEADER - 1)] + [head[-1] & ~NOTE]
                stack += [jnp.zeros_like(ref)] * (STACK - HEADER)
                unpacker[...] = jnp.stack([ref | _shl(ref, 16)] + stack)

            for side in sides:
                own_load(t, *side).wait()
            state = unpacker[...]
            ref = state[0]

            def reduce_unit(u, stack):
                words, stack = _unpack_pair(messages, both_sizes, (u, u), ref, stack)
                for j, (base, own, _) in enumerate(sides):
                    plain = messages[j][pl.ds(HEADER + u * UNIT_WORDS, UNIT_WORDS)]
                    is_plain = _tile(both_sizes[j]) == PLAIN_SIZE
                    w = [jnp.where(is_plain, plain[i], words[i][j]) for i in range(UNIT_WORDS)]
                    w = jnp.concatenate([jnp.concatenate(w[i : i + 4], axis=1) for i in range(0, 16, 4)])
                    other = pltpu.bitcast(w, jnp.bfloat16).astype(jnp.float32)
                    total = own[at(PREFETCH, t), rows(u * UNIT_ROWS, UNIT_ROWS), :] + other
                    out[rows(base + t * TICK_ROWS + u * UNIT_ROWS, UNIT_ROWS), :] = total.astype(out.dtype)
                return stack

            stack = lax.fori_loop(0, UNITS, reduce_unit, [state[1 + i] for i in range(STACK)], unroll=True)
            unpacker[...] = jnp.stack([ref] + stack)

            @pl.when(t + PREFETCH < ticks)
            def _():
                for side in sides:
                    own_load(t + PREFETCH, *side).start()

        @pl.loop(0, PREFETCH)
        def _(e):
            src_load(e).start()

        for recv in (x_recv, y_recv):
            recv[:, STREAM:] = jnp.zeros((RECV_SLOTS, PLAIN_SIZE, *TILE), I32)
        barrier = pltpu.get_barrier_semaphore()
        for peer in (x_peer, y_peer):
            pl.semaphore_signal(barrier, 1, device_id=peer, device_id_type=pl.DeviceIdType.MESH)

        @pl.loop(-2, ticks + 1)
        def _(step):
            relaying = (step >= 0) & (step < ticks)

            @pl.when(relaying)
            def _():
                head_part(step, PIECE, lambda *part: relay(step, *part))

            @pl.when(step == -1)
            def _():
                pl.semaphore_wait(barrier, 2)

            @pl.when((step >= -1) & (step + 1 < ticks))
            def _():
                start_send(step + 1)

            @pl.when(step == -1)
            def _():
                @pl.loop(0, PREFETCH)
                def _(t):
                    for side in sides:
                        own_load(t, *side).start()

            @pl.loop(0, 2)
            def _(i):
                e = packed_before(step + 2) - 2 + i
                pl.when(e >= packed_before(step + 1))(lambda: pack(e))
                pl.when(relaying)(lambda: relay(step, 1 + i, HEADER + (1 + i) * PIECE, PIECE))

            @pl.when(relaying)
            def _():
                stream_part(received_size(FROM_X, x_recv, step), lambda *part: relay(step, *part))

            @pl.when(step >= 1)
            def _():
                t = step - 1
                head_part(t, FIXED, lambda *part: y_copy(t, *part).wait())
                x_size, y_size = sizes[FROM_X, group(t)[0]], received_size(FROM_Y, y_recv, t)
                stream_part(y_size, lambda *part: y_copy(t, *part).wait_recv())
                reduce(t, (x_size, y_size))
                stream_part(x_size, lambda *part: y_copy(t, *part).wait_send())

            @pl.when(relaying)
            def _():
                head_part(step, FIXED, lambda *part: x_copy(step, *part).wait_send())
                stream_part(sizes[SENT, group(step)[0]], lambda *part: x_copy(step, *part).wait_send())

    vmem, dma = pltpu.VMEM, pltpu.SemaphoreType.DMA
    staging = vmem((PREFETCH, TICK_ROWS, n), jnp.float32)
    received = vmem((RECV_SLOTS, STREAM + PLAIN_SIZE, *TILE), I32)
    return pl.pallas_call(
        body,
        out_shape=vmem((m, n), jnp.bfloat16),
        in_specs=[pl.BlockSpec(memory_space=pl.ANY)],
        out_specs=pl.BlockSpec(memory_space=vmem),
        scratch_shapes=[
            staging, staging, staging,
            vmem((SEND_SLOTS, PLAIN_COPY + STREAM + PLAIN_SIZE, *TILE), I32),
            received, received,
            vmem((STACK + 2, *TILE), I32),
            vmem((UNITS + 1, STACK, *TILE), I32),
            vmem((STACK + 1, 2, *TILE), I32),
            pltpu.SMEM((3, ticks), I32),
            dma((PREFETCH,)), dma((PREFETCH,)), dma((PREFETCH,)),
            dma((2 * IN_FLIGHT,)), dma((4 * RECV_SLOTS,)),
            dma((2 * IN_FLIGHT,)), dma((2 * RECV_SLOTS,)),
        ],
        compiler_params=pltpu.CompilerParams(collective_id=0, vmem_limit_bytes=52 * 2**20),
    )(x)
```
